```python
import numpy as np

kernel_name = "dist_ag_xy_y_m256_n256"

def setup_inputs():
    return {"x": np.random.randn(512, 256).astype(np.float32)}

def reference(x: np.ndarray) -> np.ndarray:
    return x
```

```python
import jax
import jax.numpy as jnp
from jax import lax
from jax.experimental import pallas as pl
from jax.experimental.pallas import tpu as pltpu


def pallas_dist_ag_xy_y_m256_n256_kernel(x: jax.Array):
    m, n = x.shape

    def body(x_ref, out_ref, send_buf, recv_buf, send_sem, recv_sem):
        my_x = lax.axis_index("x")
        my_y = lax.axis_index("y")
        nbr = (my_x, 1 - my_y)
        barrier = pltpu.get_barrier_semaphore()
        pl.semaphore_signal(barrier, inc=1, device_id=nbr,
                            device_id_type=pl.DeviceIdType.MESH)
        send_buf[...] = x_ref[...].astype(jnp.bfloat16)
        pl.semaphore_wait(barrier, 1)
        rdma = pltpu.make_async_remote_copy(
            src_ref=send_buf, dst_ref=recv_buf, send_sem=send_sem,
            recv_sem=recv_sem, device_id=nbr,
            device_id_type=pl.DeviceIdType.MESH)
        rdma.start()
        out_ref[pl.ds(pl.multiple_of(my_y * m, m), m), :] = x_ref[...]
        rdma.wait_recv()
        out_ref[pl.ds(pl.multiple_of((1 - my_y) * m, m), m), :] = recv_buf[...].astype(jnp.float32)
        rdma.wait_send()

    return pl.pallas_call(
        body,
        out_shape=jax.ShapeDtypeStruct((2 * m, n), x.dtype),
        in_specs=[pl.BlockSpec(memory_space=pltpu.VMEM)],
        out_specs=pl.BlockSpec(memory_space=pltpu.VMEM),
        scratch_shapes=[
            pltpu.VMEM((m, n), jnp.bfloat16),
            pltpu.VMEM((m, n), jnp.bfloat16),
            pltpu.SemaphoreType.DMA,
            pltpu.SemaphoreType.DMA,
        ],
        compiler_params=pltpu.CompilerParams(collective_id=0),
    )(x)
```

```python
import jax
import jax.numpy as jnp
from jax import lax
from jax.experimental import pallas as pl
from jax.experimental.pallas import tpu as pltpu

_MESH = pl.DeviceIdType.MESH

_RELAY = (16, 16, 16)
_DIRECT = (144, 16)


def _offsets(chunks, start=0):
    out = [start]
    for c in chunks:
        out.append(out[-1] + c)
    return out


def pallas_dist_ag_xy_y_m256_n256_kernel(x: jax.Array):
    m, n = x.shape
    nf, nd = len(_RELAY), len(_DIRECT)
    f_rows = sum(_RELAY)
    fo = _offsets(_RELAY)
    do = _offsets(_DIRECT, f_rows)
    assert do[-1] == m - f_rows

    def body(x_ref, o_ref, xv, sb, rb, load_sems, send_sems, recv_sems, entered):
        mx, my = lax.axis_index("x"), lax.axis_index("y")
        y_nbr, x_nbr = (mx, 1 - my), (1 - mx, my)
        col0 = mx == 0
        col1 = mx != 0

        bar = pltpu.get_barrier_semaphore()
        pl.semaphore_signal(bar, inc=1, device_id=y_nbr, device_id_type=_MESH)

        @pl.when(col0)
        def _():
            pl.semaphore_signal(bar, inc=1, device_id=x_nbr, device_id_type=_MESH)

        relay0 = mx * (m - f_rows)
        miss0 = (1 - mx) * (m - f_rows)

        def rows(base, a, b):
            return pl.ds(pl.multiple_of(base + a, 16), b - a)

        parts = [rows(relay0, fo[i], fo[i + 1]) for i in range(nf)]
        parts += [pl.ds(do[i], _DIRECT[i]) for i in range(nd)]
        loads = [
            pltpu.make_async_copy(x_ref.at[s], xv.at[s], load_sems.at[i])
            for i, s in enumerate(parts + [rows(miss0, 0, f_rows)])
        ]
        for ld in loads:
            ld.start()

        sends = []
        for i, s in enumerate(parts):
            loads[i].wait()
            sb[s] = xv[s].astype(jnp.bfloat16)
            if i == 0:
                @pl.when(col0)
                def _():
                    pl.semaphore_wait(bar, 1)

                @pl.when(col1)
                def _():
                    pl.semaphore_wait(bar, 2)

            c = pltpu.make_async_remote_copy(
                sb.at[s], rb.at[s], send_sems.at[i], recv_sems.at[i],
                device_id=y_nbr, device_id_type=_MESH)
            c.start()
            sends.append(c)
            if i == 0:
                @pl.when(col1)
                def _():
                    pl.semaphore_signal(
                        entered, inc=1, device_id=x_nbr, device_id_type=_MESH)

        loads[-1].wait()
        o_ref[pl.ds(pl.multiple_of(my * m, m), m)] = xv[...]

        @pl.when(col0)
        def _():
            pl.semaphore_wait(entered, 1)

        other = (1 - my) * m
        relays = []
        for i in range(nf):
            sends[i].wait_recv()
            j = nf + nd + i
            c = pltpu.make_async_remote_copy(
                rb.at[parts[i]], rb.at[parts[i]], send_sems.at[j], recv_sems.at[j],
                device_id=x_nbr, device_id_type=_MESH)
            c.start()
            relays.append(c)
            o_ref[rows(other + relay0, fo[i], fo[i + 1])] = (
                rb[parts[i]].astype(jnp.float32))

        def finish_direct(i):
            sends[nf + i].wait_recv()
            o_ref[rows(other, do[i], do[i + 1])] = (
                rb[parts[nf + i]].astype(jnp.float32))

        def finish_relayed(i):
            s = rows(miss0, fo[i], fo[i + 1])
            j = nf + nd + i
            pltpu.make_async_remote_copy(
                rb.at[s], rb.at[s], send_sems.at[j], recv_sems.at[j],
                device_id=x_nbr, device_id_type=_MESH).wait_recv()
            o_ref[rows(other + miss0, fo[i], fo[i + 1])] = rb[s].astype(jnp.float32)

        for i in range(nd - 1):
            finish_direct(i)
        for i in range(nf - 1):
            finish_relayed(i)
        for c in sends[:-1] + relays:
            c.wait_send()
        finish_direct(nd - 1)
        finish_relayed(nf - 1)
        sends[-1].wait_send()

    n_copies = 2 * nf + nd
    return pl.pallas_call(
        body,
        out_shape=jax.ShapeDtypeStruct((2 * m, n), x.dtype),
        in_specs=[pl.BlockSpec(memory_space=pltpu.MemorySpace.HBM)],
        out_specs=pl.BlockSpec(memory_space=pltpu.MemorySpace.VMEM),
        scratch_shapes=[
            pltpu.VMEM((m, n), jnp.float32),
            pltpu.VMEM((m, n), jnp.bfloat16),
            pltpu.VMEM((m, n), jnp.bfloat16),
            pltpu.SemaphoreType.DMA((nf + nd + 1,)),
            pltpu.SemaphoreType.DMA((n_copies,)),
            pltpu.SemaphoreType.DMA((n_copies,)),
            pltpu.SemaphoreType.REGULAR,
        ],
        compiler_params=pltpu.CompilerParams(collective_id=0),
    )(x)
```
